```python
import numpy as np

kernel_name = "dist_redx_gaty_m512_n512"

def setup_inputs():
    return {"x": np.random.randn(1024, 1024).astype(np.float32)}

def reference(x: np.ndarray) -> np.ndarray:
    return x.reshape(2, 512, 1024).sum(axis=0)
```

```python
import jax
import jax.numpy as jnp
from jax import lax
from jax.experimental import pallas as pl
from jax.experimental.pallas import tpu as pltpu

MESH = pl.DeviceIdType.MESH
F32, BF16, I32 = jnp.float32, jnp.bfloat16, jnp.int32

M = 512
N = 512
CH = 16
K = M // CH
NR = 4
KS = K - NR
LAST = KS - 1
FLAG = KS - 2
EARLY = 12
LAG = 8
FWD_AT = KS - EARLY + 1
HALF = N // 2

SLOT = 32
HDR = 24
ESC_A, ESC_B = 14 << 7, 15 << 7
LEVEL_SHIFT = 16
RAW_BAD, SUM_BAD = 2 << LEVEL_SHIFT, 1 << LEVEL_SHIFT

_LOADS = [[0], [1], [2, 3], [4, 5], list(range(KS, K))]
_LOADS += [list(range(p, min(p + 4, KS))) for p in range(6, KS, 4)]
_LOAD_OF = {p: i for i, g in enumerate(_LOADS) for p in g}


def _x_header(p):
    return (p, 0) if p in (1, FLAG, LAST) or p % 2 == 0 else (p - 1, 1)


def _y_header(p):
    if p >= KS:
        return _x_header(p)
    return (p, 0) if p == FLAG else (p | 1, p % 2)


def _srl(x, n):
    return lax.shift_right_logical(x, jnp.broadcast_to(jnp.asarray(n, I32), x.shape))


def _sll(x, n):
    return lax.shift_left(x, jnp.broadcast_to(jnp.asarray(n, I32), x.shape))


def _to_tiles(v):
    n = v.shape[1] // 128
    return jnp.stack([v[8 * r:8 * r + 8, 128 * c:128 * c + 128]
                      for r in range(2) for c in range(n)])


def _from_tiles(t):
    n = t.shape[0] // 2
    return jnp.concatenate(
        [jnp.concatenate([t[n * r + c] for c in range(n)], axis=1) for r in range(2)], axis=0)


def _pack(v, bad):
    tile = lax.broadcasted_iota(I32, (8, 8, 128), 0)
    t = lax.bitcast_convert_type(_to_tiles(v).astype(BF16).astype(F32), I32)
    h = _srl(t, 16) & 0x7FFF
    top = jnp.max(jnp.max(h, axis=0), axis=0, keepdims=True) | 0x7F
    bot = jnp.min(jnp.min(h, axis=0), axis=0, keepdims=True) | 0x7F
    code = top[None] - h
    far = code >= ESC_A
    esc = jnp.max(jnp.max(jnp.where(far, h, 0), axis=0), axis=0, keepdims=True) & 0x7F80
    is_esc = h >= esc[None]
    lost = far & jnp.logical_not(is_esc) & ((h | 0x7F) != bot[None])
    code = jnp.where(far, jnp.where(is_esc, ESC_A, ESC_B) | (code & 0x7F), code)
    byte = _sll(code & 0xFF, (tile & 3) * 8)
    nib = _sll(_srl(code, 8) | (_srl(t, 28) & 8), tile * 4)
    planes = jnp.concatenate(
        [jnp.sum(byte[:4], axis=0), jnp.sum(byte[4:], axis=0), jnp.sum(nib, axis=0)], axis=0)
    top_e = _srl(top, 7)

    def distance(x):
        e = _srl(x, 7)
        d = jnp.where(e == 0, 15, jnp.maximum(top_e - 14 - e, 0))
        return jnp.minimum(d, 15), jnp.logical_and(e > 0, d > 14)

    (esc_d, esc_lost), (bot_d, bot_lost) = distance(esc), distance(bot)
    lane_lost = jnp.logical_or(esc_lost, bot_lost).astype(I32)
    bad = jnp.maximum(jnp.maximum(bad, jnp.max(lost.astype(I32), axis=0)), lane_lost)
    return planes, top_e | _sll(esc_d, 8) | _sll(bot_d, 12), bad


def _unpack(planes, hdr):
    tile = lax.broadcasted_iota(I32, (8, 8, 128), 0)
    byte = jnp.stack([planes[0:8]] * 4 + [planes[8:16]] * 4)
    nib = _srl(jnp.stack([planes[16:24]] * 8), tile * 4)
    top_e = hdr & 0xFF

    def base(shift, escape):
        d = _srl(hdr, shift) & 15
        e = jnp.where(d == 15, 0, top_e - 14 - d)
        return ((_sll(e, 7) | 0x7F) + escape)[None]

    code = (_srl(byte, (tile & 3) * 8) & 0xFF) | _sll(nib & 7, 8)
    h = jnp.where(code >= ESC_A,
                  jnp.where(code >= ESC_B, base(12, ESC_B), base(8, ESC_A)),
                  (_sll(top_e, 7) | 0x7F)[None]) - code
    return _from_tiles(lax.bitcast_convert_type(_sll(h, 16) | _sll(nib & 8, 28), F32))


def _lane_level(bad, value):
    return jnp.where(jnp.max(bad, axis=0, keepdims=True) > 0, value, 0)


def _body(x_hbm, out, xin, xw, xr, yw, yr, fw, x0l, x0s, x0r, yls, ylr,
          xs16, xr16, ys16, yr16,
          in_sems, xr_sems, yr_sems, fw_sems, send_sems, p0_sems, slow_sems, dsem):
    mx = lax.axis_index("x")
    my = lax.axis_index("y")
    xn = (1 - mx, my)
    yn = (mx, 1 - my)
    is_a = jnp.logical_and(mx == 0, my == 0)
    is_b = jnp.logical_and(mx == 0, my == 1)
    is_c = jnp.logical_and(mx == 1, my == 0)
    is_d = jnp.logical_and(mx == 1, my == 1)
    own = pl.ds(pl.multiple_of(my * N, N), N)
    oth = pl.ds(pl.multiple_of((1 - my) * N, N), N)

    def rows(p, n=1):
        return pl.ds(p * CH, n * CH)

    def slot(p, header):
        return pl.ds(p * SLOT, HDR + (header(p)[0] == p))

    def read(ref, q, p, header):
        holder, half = header(p)
        row = ref[pl.ds((q + holder - p) * SLOT + HDR, 1), :]
        return _unpack(ref[pl.ds(q * SLOT, HDR), :], _srl(row, 16 * half) & 0xFFFF)

    def remote(src, dst, send_sem, recv_sem, dev):
        return pltpu.make_async_remote_copy(src, dst, send_sem, recv_sem,
                                            device_id=dev, device_id_type=MESH)

    def x_copy(p):
        return remote(xw.at[slot(p, _x_header)], xr.at[slot(p, _x_header)], send_sems.at[0],
                      xr_sems.at[p], xn)

    def y_copy(p):
        if p == LAST:
            return remote(yls, ylr, send_sems.at[3], yr_sems.at[p], yn)
        src = yw if p < KS else xw
        return remote(src.at[slot(p, _y_header)], yr.at[slot(p, _y_header)], send_sems.at[1],
                      yr_sems.at[p], yn)

    def fw_copy(p):
        dst = pl.ds((p - KS) * SLOT, HDR + (_x_header(p)[0] == p))
        return remote(yr.at[slot(p, _x_header)], fw.at[dst], send_sems.at[2],
                      fw_sems.at[p - KS], xn)

    p0a = remote(x_hbm.at[rows(0), pl.ds(0, HALF)], x0l, p0_sems.at[0], p0_sems.at[1], xn)
    p0b = remote(x0s, x0r, p0_sems.at[2], p0_sems.at[3], xn)

    def start_x(ps):
        for p in ps:
            if p == 0:
                p0a.start()
                p0b.start()
            else:
                x_copy(p).start()

    def start_raw():
        for p in range(KS, K):
            y_copy(p).start()

    loads = [pltpu.make_async_copy(x_hbm.at[rows(g[0], len(g))], xin.at[rows(g[0], len(g))],
                                   in_sems.at[i]) for i, g in enumerate(_LOADS)]
    bar = pltpu.get_barrier_semaphore()

    @pl.when(is_c)
    def _():
        pl.semaphore_wait(bar, 1)
        p0a.start()

    loads[0].start()

    @pl.when(jnp.logical_not(is_d))
    def _():
        pl.semaphore_signal(bar, inc=1, device_id=xn, device_id_type=MESH)
        pl.semaphore_signal(bar, inc=1, device_id=yn, device_id_type=MESH)

    for ld in loads[1:]:
        ld.start()

    @pl.when(is_d)
    def _():
        pl.semaphore_wait(bar, 2)
        pl.semaphore_signal(dsem, inc=1, device_id=yn, device_id_type=MESH)
        pl.semaphore_signal(dsem, inc=1, device_id=xn, device_id_type=MESH)
        p0a.start()

    loaded = set()

    def need(p):
        if _LOAD_OF[p] not in loaded:
            loaded.add(_LOAD_OF[p])
            loads[_LOAD_OF[p]].wait()

    def encode_x(ps, bad):
        packed = []
        for p in ps:
            need(p)
            planes, hdr, bad = _pack(xin[rows(p), :], bad)
            packed.append((planes, hdr))
        hdr = packed[0][1]
        if len(ps) == 2:
            hdr = hdr | _sll(packed[1][1], 16)
            xw[pl.ds(ps[1] * SLOT, HDR), :] = packed[1][0]
        elif ps[0] == FLAG:
            hdr = hdr | _lane_level(bad, RAW_BAD)
        xw[pl.ds(ps[0] * SLOT, HDR + 1), :] = jnp.concatenate([packed[0][0], hdr], axis=0)
        return bad

    need(0)
    x0s[...] = xin[rows(0), pl.ds(HALF, HALF)].astype(BF16)

    @pl.when(mx == 1)
    def _():
        p0b.start()

    bad_x = jnp.zeros((8, 128), I32)
    batches = [[1], [2, 3], [4, 5], list(range(KS, K))]
    batches += [list(range(p, min(p + 4, EARLY))) for p in range(6, EARLY, 4)]
    for batch in batches:
        for i in range(0, len(batch), 2):
            bad_x = encode_x(batch[i:i + 2], bad_x)
        if batch[0] < KS:
            @pl.when(mx == 1)
            def _():
                start_x(batch)
        else:
            @pl.when(is_d)
            def _():
                start_raw()

            @pl.when(is_b)
            def _():
                pl.semaphore_wait(bar, 1)
                start_raw()

    @pl.when(is_a)
    def _():
        pl.semaphore_wait(bar, 2)
        start_x([0, 1])
        start_raw()
        start_x(range(2, EARLY))

    @pl.when(is_b)
    def _():
        pl.semaphore_wait(dsem, 1)
        start_x(range(EARLY))

    @pl.when(is_c)
    def _():
        pl.semaphore_wait(dsem, 1)
        start_raw()

    def finish_y(ps):
        for p in ps:
            y_copy(p).wait_recv()
        for p in ps:
            store_y(p)

    def store_y(p):
        got = ylr[...].astype(F32) if p == LAST else read(yr, p, p, _y_header)
        out[rows(p), oth] = got

    def finish_fw(p):
        fw_copy(p).wait_recv()
        out[rows(p), oth] = read(yr, p, p, _x_header) + read(fw, p - KS, p, _x_header)

    def level_of(ref):
        hdr = ref[pl.ds(FLAG * SLOT + HDR, 1), :]
        return jnp.max(_srl(hdr, LEVEL_SHIFT).astype(F32))

    late = [[p, p + 1] for p in range(EARLY, FLAG, 2)] + [[LAST], [FLAG]]
    encoded, next_x, next_y = set(range(EARLY)), EARLY, 0
    bad_y = jnp.zeros((8, 128), I32)
    my_level = held = None
    for p in range(K):
        mine = xin[rows(p), :]
        if p == 0:
            p0a.wait_recv()
            p0b.wait_recv()
            got = jnp.concatenate([x0l[...], x0r[...].astype(F32)], axis=1)
        else:
            x_copy(p).wait_recv()
            got = read(xr, p, p, _x_header)
        s = mine + got
        if p == LAST:
            yls[...] = s.astype(BF16)
        elif p < KS:
            planes, hdr, bad_y = _pack(s, bad_y)
            if p == FLAG:
                hdr_row = pl.ds(p * SLOT + HDR, 1)
                raw_level = (xw[hdr_row, :] | xr[hdr_row, :]) & RAW_BAD
                hdr = hdr | jnp.maximum(_lane_level(bad_y, SUM_BAD), raw_level)
            elif p % 2 == 0:
                held, hdr = hdr, None
            else:
                hdr = held | _sll(hdr, 16)
            if hdr is None:
                yw[pl.ds(p * SLOT, HDR), :] = planes
            else:
                yw[pl.ds(p * SLOT, HDR + 1), :] = jnp.concatenate([planes, hdr], axis=0)
        if p < KS:
            y_copy(p).start()
        out[rows(p), own] = s

        if late and (p % 2 == 0 or len(late[0]) == 1):
            ps = late.pop(0)
            bad_x = encode_x(ps, bad_x)
            encoded.update(ps)
            while next_x in encoded:
                x_copy(next_x).start()
                next_x += 1
            if not late:
                start_x(range(KS, K))
        if p == FWD_AT:
            assert not late
            for q in range(KS, K):
                y_copy(q).wait_recv()
                fw_copy(q).start()
        if next_y < FLAG and next_y + 1 <= p - LAG:
            finish_y([next_y, next_y + 1])
            next_y += 2
        if p == FLAG + 1:
            my_level = level_of(yw)

    for p in range(next_y, FLAG, 2):
        finish_y([p, p + 1])
    finish_y([FLAG])
    in_level = level_of(yr)
    for p in range(KS, K - 1):
        finish_fw(p)
    p0a.wait_send()
    p0b.wait_send()
    for p in range(1, K):
        x_copy(p).wait_send()
    for p in range(K):
        y_copy(p).wait_send()
    for p in range(KS, K):
        fw_copy(p).wait_send()
    finish_fw(K - 1)
    finish_y([LAST])

    raw_bad = jnp.maximum(my_level, in_level) >= 2
    send_y = jnp.logical_or(raw_bad, my_level > 0)
    recv_y = jnp.logical_or(raw_bad, in_level > 0)

    @pl.when(jnp.logical_or(send_y, recv_y))
    def _():
        slow_x = remote(xs16, xr16, slow_sems.at[0], slow_sems.at[1], xn)
        slow_y = remote(ys16, yr16, slow_sems.at[2], slow_sems.at[3], yn)

        @pl.when(raw_bad)
        def _():
            xs16[...] = xin[...].astype(BF16)
            slow_x.start()
            slow_x.wait()
            out[:, own] = xin[...] + xr16[...].astype(F32)

        @pl.when(send_y)
        def _():
            ys16[...] = out[:, own].astype(BF16)
            slow_y.start()

        @pl.when(recv_y)
        def _():
            slow_y.wait_recv()
            out[:, oth] = yr16[...].astype(F32)

        @pl.when(send_y)
        def _():
            slow_y.wait_send()


def pallas_dist_redx_gaty_m512_n512_kernel(x: jax.Array):
    dma = pltpu.SemaphoreType.DMA

    def wire(n):
        return pltpu.VMEM((n * SLOT, 128), I32)

    def plain(r, c):
        return pltpu.VMEM((r, c), BF16)

    return pl.pallas_call(
        _body,
        out_shape=pltpu.VMEM((M, 2 * N), F32),
        in_specs=[pl.BlockSpec(memory_space=pl.ANY)],
        out_specs=pl.BlockSpec(memory_space=pltpu.VMEM),
        scratch_shapes=[
            pltpu.VMEM((M, N), F32),
            wire(K), wire(K), wire(KS), wire(K), wire(NR),
            pltpu.VMEM((CH, HALF), F32), plain(CH, HALF), plain(CH, HALF),
            plain(CH, N), plain(CH, N),
            plain(M, N), plain(M, N), plain(M, N), plain(M, N),
            dma((len(_LOADS),)), dma((K,)), dma((K,)), dma((NR,)), dma((4,)),
            dma((4,)), dma((4,)), pltpu.SemaphoreType.REGULAR,
        ],
        compiler_params=pltpu.CompilerParams(collective_id=0, disable_semaphore_checks=True),
    )(x)
```

```python
import jax
import jax.numpy as jnp
from jax import lax
from jax.experimental import pallas as pl
from jax.experimental.pallas import tpu as pltpu

MESH = pl.DeviceIdType.MESH
F32, BF16, I32 = jnp.float32, jnp.bfloat16, jnp.int32

M = 512
N = 512
CH = 16
K = M // CH
NR = 4
KS = K - NR
LAST = KS - 1
FLAG = KS - 2
EARLY = 12
LAG = 8
FWD_AT = KS - EARLY + 1
HALF = N // 2

SLOT = 32
HDR = 24
ESC_A, ESC_B = 14 << 7, 15 << 7
LEVEL_SHIFT = 16
RAW_BAD, SUM_BAD = 2 << LEVEL_SHIFT, 1 << LEVEL_SHIFT

_LOADS = [[0], [1], [2, 3], [4, 5], list(range(KS, K))]
_LOADS += [list(range(p, min(p + 4, KS))) for p in range(6, KS, 4)]
_LOAD_OF = {p: i for i, g in enumerate(_LOADS) for p in g}


def _x_header(p):
    return (p, 0) if p in (1, FLAG, LAST) or p % 2 == 0 else (p - 1, 1)


def _y_header(p):
    if p >= KS:
        return _x_header(p)
    return (p, 0) if p == FLAG else (p | 1, p % 2)


def _srl(x, n):
    return lax.shift_right_logical(x, jnp.broadcast_to(jnp.asarray(n, I32), x.shape))


def _sll(x, n):
    return lax.shift_left(x, jnp.broadcast_to(jnp.asarray(n, I32), x.shape))


def _to_tiles(v):
    n = v.shape[1] // 128
    return jnp.stack([v[8 * r:8 * r + 8, 128 * c:128 * c + 128]
                      for r in range(2) for c in range(n)])


def _from_tiles(t):
    n = t.shape[0] // 2
    return jnp.concatenate(
        [jnp.concatenate([t[n * r + c] for c in range(n)], axis=1) for r in range(2)], axis=0)


def _pack(v, bad):
    tile = lax.broadcasted_iota(I32, (8, 8, 128), 0)
    t = lax.bitcast_convert_type(_to_tiles(v).astype(BF16).astype(F32), I32)
    h = _srl(t, 16) & 0x7FFF
    top = jnp.max(jnp.max(h, axis=0), axis=0, keepdims=True) | 0x7F
    bot = jnp.min(jnp.min(h, axis=0), axis=0, keepdims=True) | 0x7F
    code = top[None] - h
    far = code >= ESC_A
    esc = jnp.max(jnp.max(jnp.where(far, h, 0), axis=0), axis=0, keepdims=True) & 0x7F80
    is_esc = h >= esc[None]
    lost = far & jnp.logical_not(is_esc) & ((h | 0x7F) != bot[None])
    code = jnp.where(far, jnp.where(is_esc, ESC_A, ESC_B) | (code & 0x7F), code)
    byte = _sll(code & 0xFF, (tile & 3) * 8)
    nib = _sll(_srl(code, 8) | (_srl(t, 28) & 8), tile * 4)
    planes = jnp.concatenate(
        [jnp.sum(byte[:4], axis=0), jnp.sum(byte[4:], axis=0), jnp.sum(nib, axis=0)], axis=0)
    top_e = _srl(top, 7)

    def distance(x):
        e = _srl(x, 7)
        d = jnp.where(e == 0, 15, jnp.maximum(top_e - 14 - e, 0))
        return jnp.minimum(d, 15), jnp.logical_and(e > 0, d > 14)

    (esc_d, esc_lost), (bot_d, bot_lost) = distance(esc), distance(bot)
    lane_lost = jnp.logical_or(esc_lost, bot_lost).astype(I32)
    bad = jnp.maximum(jnp.maximum(bad, jnp.max(lost.astype(I32), axis=0)), lane_lost)
    return planes, top_e | _sll(esc_d, 8) | _sll(bot_d, 12), bad


def _unpack(planes, hdr):
    tile = lax.broadcasted_iota(I32, (8, 8, 128), 0)
    byte = jnp.stack([planes[0:8]] * 4 + [planes[8:16]] * 4)
    nib = _srl(jnp.stack([planes[16:24]] * 8), tile * 4)
    top_e = hdr & 0xFF

    def base(shift, escape):
        d = _srl(hdr, shift) & 15
        e = jnp.where(d == 15, 0, top_e - 14 - d)
        return ((_sll(e, 7) | 0x7F) + escape)[None]

    code = (_srl(byte, (tile & 3) * 8) & 0xFF) | _sll(nib & 7, 8)
    h = jnp.where(code >= ESC_A,
                  jnp.where(code >= ESC_B, base(12, ESC_B), base(8, ESC_A)),
                  (_sll(top_e, 7) | 0x7F)[None]) - code
    return _from_tiles(lax.bitcast_convert_type(_sll(h, 16) | _sll(nib & 8, 28), F32))


def _lane_level(bad, value):
    return jnp.where(jnp.max(bad, axis=0, keepdims=True) > 0, value, 0)


def _body(x_hbm, out, xin, xw, xr, yw, yr, fw, x0l, x0s, x0r, yls, ylr,
          xs16, xr16, ys16, yr16,
          in_sems, xr_sems, yr_sems, fw_sems, send_sems, p0_sems, slow_sems, dsem):
    mx = lax.axis_index("x")
    my = lax.axis_index("y")
    xn = (1 - mx, my)
    yn = (mx, 1 - my)
    is_a = jnp.logical_and(mx == 0, my == 0)
    is_b = jnp.logical_and(mx == 0, my == 1)
    is_c = jnp.logical_and(mx == 1, my == 0)
    is_d = jnp.logical_and(mx == 1, my == 1)
    own = pl.ds(pl.multiple_of(my * N, N), N)
    oth = pl.ds(pl.multiple_of((1 - my) * N, N), N)

    def rows(p, n=1):
        return pl.ds(p * CH, n * CH)

    def slot(p, header):
        return pl.ds(p * SLOT, HDR + (header(p)[0] == p))

    def read(ref, q, p, header):
        holder, half = header(p)
        row = ref[pl.ds((q + holder - p) * SLOT + HDR, 1), :]
        return _unpack(ref[pl.ds(q * SLOT, HDR), :], _srl(row, 16 * half) & 0xFFFF)

    def remote(src, dst, send_sem, recv_sem, dev):
        return pltpu.make_async_remote_copy(src, dst, send_sem, recv_sem,
                                            device_id=dev, device_id_type=MESH)

    def x_copy(p):
        return remote(xw.at[slot(p, _x_header)], xr.at[slot(p, _x_header)], send_sems.at[0],
                      xr_sems.at[p], xn)

    def y_copy(p):
        if p == LAST:
            return remote(yls, ylr, send_sems.at[3], yr_sems.at[p], yn)
        src = yw if p < KS else xw
        return remote(src.at[slot(p, _y_header)], yr.at[slot(p, _y_header)], send_sems.at[1],
                      yr_sems.at[p], yn)

    def fw_copy(p):
        dst = pl.ds((p - KS) * SLOT, HDR + (_x_header(p)[0] == p))
        return remote(yr.at[slot(p, _x_header)], fw.at[dst], send_sems.at[2],
                      fw_sems.at[p - KS], xn)

    p0a = remote(x_hbm.at[rows(0), pl.ds(0, HALF)], x0l, p0_sems.at[0], p0_sems.at[1], xn)
    p0b = remote(x0s, x0r, p0_sems.at[2], p0_sems.at[3], xn)

    def start_x(ps):
        for p in ps:
            if p == 0:
                p0a.start()
                p0b.start()
            else:
                x_copy(p).start()

    def start_raw():
        for p in range(KS, K):
            y_copy(p).start()

    loads = [pltpu.make_async_copy(x_hbm.at[rows(g[0], len(g))], xin.at[rows(g[0], len(g))],
                                   in_sems.at[i]) for i, g in enumerate(_LOADS)]
    bar = pltpu.get_barrier_semaphore()

    @pl.when(is_c)
    def _():
        pl.semaphore_wait(bar, 1)
        p0a.start()

    loads[0].start()

    @pl.when(jnp.logical_not(is_d))
    def _():
        pl.semaphore_signal(bar, inc=1, device_id=xn, device_id_type=MESH)
        pl.semaphore_signal(bar, inc=1, device_id=yn, device_id_type=MESH)

    for ld in loads[1:]:
        ld.start()

    @pl.when(is_d)
    def _():
        pl.semaphore_wait(bar, 2)
        pl.semaphore_signal(dsem, inc=1, device_id=yn, device_id_type=MESH)
        pl.semaphore_signal(dsem, inc=1, device_id=xn, device_id_type=MESH)
        p0a.start()

    loaded = set()

    def need(p):
        if _LOAD_OF[p] not in loaded:
            loaded.add(_LOAD_OF[p])
            loads[_LOAD_OF[p]].wait()

    def encode_x(ps, bad):
        packed = []
        for p in ps:
            need(p)
            planes, hdr, bad = _pack(xin[rows(p), :], bad)
            packed.append((planes, hdr))
        hdr = packed[0][1]
        if len(ps) == 2:
            hdr = hdr | _sll(packed[1][1], 16)
            xw[pl.ds(ps[1] * SLOT, HDR), :] = packed[1][0]
        elif ps[0] == FLAG:
            hdr = hdr | _lane_level(bad, RAW_BAD)
        xw[pl.ds(ps[0] * SLOT, HDR + 1), :] = jnp.concatenate([packed[0][0], hdr], axis=0)
        return bad

    need(0)
    x0s[...] = xin[rows(0), pl.ds(HALF, HALF)].astype(BF16)

    @pl.when(mx == 1)
    def _():
        p0b.start()

    bad_x = jnp.zeros((8, 128), I32)
    batches = [[1], [2, 3], [4, 5], list(range(KS, K))]
    batches += [list(range(p, min(p + 4, EARLY))) for p in range(6, EARLY, 4)]
    for batch in batches:
        for i in range(0, len(batch), 2):
            bad_x = encode_x(batch[i:i + 2], bad_x)
        if batch[0] < KS:
            @pl.when(mx == 1)
            def _():
                start_x(batch)
        else:
            @pl.when(is_d)
            def _():
                start_raw()

            @pl.when(is_b)
            def _():
                pl.semaphore_wait(bar, 1)
                start_raw()

    @pl.when(is_a)
    def _():
        pl.semaphore_wait(bar, 2)
        start_x([0, 1])
        start_raw()
        start_x(range(2, EARLY))

    @pl.when(is_b)
    def _():
        pl.semaphore_wait(dsem, 1)
        start_x(range(EARLY))

    @pl.when(is_c)
    def _():
        pl.semaphore_wait(dsem, 1)
        start_raw()

    def finish_y(ps):
        for p in ps:
            y_copy(p).wait_recv()
        for p in ps:
            store_y(p)

    def store_y(p):
        got = ylr[...].astype(F32) if p == LAST else read(yr, p, p, _y_header)
        out[rows(p), oth] = got

    def finish_fw(p):
        fw_copy(p).wait_recv()
        out[rows(p), oth] = out[rows(p), oth] + read(fw, p - KS, p, _x_header)

    def level_of(ref):
        hdr = ref[pl.ds(FLAG * SLOT + HDR, 1), :]
        return jnp.max(_srl(hdr, LEVEL_SHIFT).astype(F32))

    late = [[p, p + 1] for p in range(EARLY, FLAG, 2)] + [[LAST], [FLAG]]
    encoded, next_x, next_y = set(range(EARLY)), EARLY, 0
    bad_y = jnp.zeros((8, 128), I32)
    my_level = held = None
    for p in range(K):
        mine = xin[rows(p), :]
        if p == 0:
            p0a.wait_recv()
            p0b.wait_recv()
            got = jnp.concatenate([x0l[...], x0r[...].astype(F32)], axis=1)
        else:
            x_copy(p).wait_recv()
            got = read(xr, p, p, _x_header)
        s = mine + got
        if p == LAST:
            yls[...] = s.astype(BF16)
        elif p < KS:
            planes, hdr, bad_y = _pack(s, bad_y)
            if p == FLAG:
                hdr_row = pl.ds(p * SLOT + HDR, 1)
                raw_level = (xw[hdr_row, :] | xr[hdr_row, :]) & RAW_BAD
                hdr = hdr | jnp.maximum(_lane_level(bad_y, SUM_BAD), raw_level)
            elif p % 2 == 0:
                held, hdr = hdr, None
            else:
                hdr = held | _sll(hdr, 16)
            if hdr is None:
                yw[pl.ds(p * SLOT, HDR), :] = planes
            else:
                yw[pl.ds(p * SLOT, HDR + 1), :] = jnp.concatenate([planes, hdr], axis=0)
        if p < KS:
            y_copy(p).start()
        out[rows(p), own] = s

        if late and (p % 2 == 0 or len(late[0]) == 1):
            ps = late.pop(0)
            bad_x = encode_x(ps, bad_x)
            encoded.update(ps)
            while next_x in encoded:
                x_copy(next_x).start()
                next_x += 1
            if not late:
                start_x(range(KS, K))
        if p == FWD_AT:
            assert not late
            for q in range(KS, K):
                y_copy(q).wait_recv()
                fw_copy(q).start()
            for q in range(KS, K):
                out[rows(q), oth] = read(yr, q, q, _x_header)
        if next_y < FLAG and next_y + 1 <= p - LAG:
            finish_y([next_y, next_y + 1])
            next_y += 2
        if p == FLAG + 1:
            my_level = level_of(yw)

    finish_fw(KS)
    for p in range(next_y, FLAG, 2):
        finish_y([p, p + 1])
    for p in range(KS + 1, K - 1):
        finish_fw(p)
    finish_y([FLAG])
    in_level = level_of(yr)
    p0a.wait_send()
    p0b.wait_send()
    for p in range(1, K):
        x_copy(p).wait_send()
    for p in range(K):
        y_copy(p).wait_send()
    for p in range(KS, K):
        fw_copy(p).wait_send()
    finish_fw(K - 1)
    finish_y([LAST])

    raw_bad = jnp.maximum(my_level, in_level) >= 2
    send_y = jnp.logical_or(raw_bad, my_level > 0)
    recv_y = jnp.logical_or(raw_bad, in_level > 0)

    @pl.when(jnp.logical_or(send_y, recv_y))
    def _():
        slow_x = remote(xs16, xr16, slow_sems.at[0], slow_sems.at[1], xn)
        slow_y = remote(ys16, yr16, slow_sems.at[2], slow_sems.at[3], yn)

        @pl.when(raw_bad)
        def _():
            xs16[...] = xin[...].astype(BF16)
            slow_x.start()
            slow_x.wait()
            out[:, own] = xin[...] + xr16[...].astype(F32)

        @pl.when(send_y)
        def _():
            ys16[...] = out[:, own].astype(BF16)
            slow_y.start()

        @pl.when(recv_y)
        def _():
            slow_y.wait_recv()
            out[:, oth] = yr16[...].astype(F32)

        @pl.when(send_y)
        def _():
            slow_y.wait_send()


def pallas_dist_redx_gaty_m512_n512_kernel(x: jax.Array):
    dma = pltpu.SemaphoreType.DMA

    def wire(n):
        return pltpu.VMEM((n * SLOT, 128), I32)

    def plain(r, c):
        return pltpu.VMEM((r, c), BF16)

    return pl.pallas_call(
        _body,
        out_shape=pltpu.VMEM((M, 2 * N), F32),
        in_specs=[pl.BlockSpec(memory_space=pl.ANY)],
        out_specs=pl.BlockSpec(memory_space=pltpu.VMEM),
        scratch_shapes=[
            pltpu.VMEM((M, N), F32),
            wire(K), wire(K), wire(KS), wire(K), wire(NR),
            pltpu.VMEM((CH, HALF), F32), plain(CH, HALF), plain(CH, HALF),
            plain(CH, N), plain(CH, N),
            plain(M, N), plain(M, N), plain(M, N), plain(M, N),
            dma((len(_LOADS),)), dma((K,)), dma((K,)), dma((NR,)), dma((4,)),
            dma((4,)), dma((4,)), pltpu.SemaphoreType.REGULAR,
        ],
        compiler_params=pltpu.CompilerParams(collective_id=0, disable_semaphore_checks=True),
    )(x)
```

```python
import jax
import jax.numpy as jnp
from jax import lax
from jax.experimental import pallas as pl
from jax.experimental.pallas import tpu as pltpu

MESH = pl.DeviceIdType.MESH
F32, BF16, I32 = jnp.float32, jnp.bfloat16, jnp.int32

M = 512
N = 512
CH = 16
K = M // CH
NR = 4
KS = K - NR
LAST = KS - 1
FLAG = KS - 2
EARLY = 12
LAG = 10
FWD_AT = KS - EARLY + 1
HALF = N // 2

SLOT = 32
HDR = 24
ESC_A, ESC_B = 14 << 7, 15 << 7
LEVEL_SHIFT = 16
RAW_BAD, SUM_BAD = 2 << LEVEL_SHIFT, 1 << LEVEL_SHIFT

_LOADS = [[0], [1], [2, 3], [4, 5], list(range(KS, K))]
_LOADS += [list(range(p, min(p + 4, KS))) for p in range(6, KS, 4)]
_LOAD_OF = {p: i for i, g in enumerate(_LOADS) for p in g}


def _x_header(p):
    return (p, 0) if p in (1, FLAG, LAST) or p % 2 == 0 else (p - 1, 1)


def _y_header(p):
    if p >= KS:
        return _x_header(p)
    return (p, 0) if p == FLAG else (p | 1, p % 2)


def _srl(x, n):
    return lax.shift_right_logical(x, jnp.broadcast_to(jnp.asarray(n, I32), x.shape))


def _sll(x, n):
    return lax.shift_left(x, jnp.broadcast_to(jnp.asarray(n, I32), x.shape))


def _to_tiles(v):
    n = v.shape[1] // 128
    return jnp.stack([v[8 * r:8 * r + 8, 128 * c:128 * c + 128]
                      for r in range(2) for c in range(n)])


def _from_tiles(t):
    n = t.shape[0] // 2
    return jnp.concatenate(
        [jnp.concatenate([t[n * r + c] for c in range(n)], axis=1) for r in range(2)], axis=0)


def _pack(v, bad):
    tile = lax.broadcasted_iota(I32, (8, 8, 128), 0)
    t = lax.bitcast_convert_type(_to_tiles(v).astype(BF16).astype(F32), I32)
    h = _srl(t, 16) & 0x7FFF
    top = jnp.max(jnp.max(h, axis=0), axis=0, keepdims=True) | 0x7F
    bot = jnp.min(jnp.min(h, axis=0), axis=0, keepdims=True) | 0x7F
    code = top[None] - h
    far = code >= ESC_A
    esc = jnp.max(jnp.max(jnp.where(far, h, 0), axis=0), axis=0, keepdims=True) & 0x7F80
    top_e, esc_e, bot_e = _srl(top, 7), _srl(esc, 7), _srl(bot, 7)
    esc_d = jnp.where(esc_e == 0, 7, top_e - 14 - esc_e)
    bot_d = jnp.where(bot_e == 0, 31, jnp.maximum(top_e - 14 - bot_e, 0))
    esc = jnp.where(jnp.logical_and(esc_e > 0, esc_d > 6), 0x8000, esc)
    bot_lost = jnp.logical_and(bot_e > 0, bot_d > 30)
    is_esc = h >= esc[None]
    lost = far & jnp.logical_not(is_esc) & ((h | 0x7F) != bot[None])
    bad = jnp.maximum(jnp.maximum(bad, jnp.max(lost.astype(I32), axis=0)), bot_lost.astype(I32))
    code = jnp.where(far, jnp.where(is_esc, ESC_A, ESC_B) | (code & 0x7F), code)
    byte = _sll(code & 0xFF, (tile & 3) * 8)
    nib = _sll(_srl(code, 8) | (_srl(t, 28) & 8), tile * 4)
    planes = jnp.concatenate(
        [jnp.sum(byte[:4], axis=0), jnp.sum(byte[4:], axis=0), jnp.sum(nib, axis=0)], axis=0)
    hdr = top_e | _sll(jnp.minimum(esc_d, 7), 8) | _sll(jnp.minimum(bot_d, 31), 11)
    return planes, hdr, bad


def _unpack(planes, hdr):
    tile = lax.broadcasted_iota(I32, (8, 8, 128), 0)
    byte = jnp.stack([planes[0:8]] * 4 + [planes[8:16]] * 4)
    nib = _srl(jnp.stack([planes[16:24]] * 8), tile * 4)
    top_e = hdr & 0xFF

    def base(shift, ones, escape):
        d = _srl(hdr, shift) & ones
        e = jnp.where(d == ones, 0, top_e - 14 - d)
        return ((_sll(e, 7) | 0x7F) + escape)[None]

    code = (_srl(byte, (tile & 3) * 8) & 0xFF) | _sll(nib & 7, 8)
    h = jnp.where(code >= ESC_A,
                  jnp.where(code >= ESC_B, base(11, 31, ESC_B), base(8, 7, ESC_A)),
                  (_sll(top_e, 7) | 0x7F)[None]) - code
    return _from_tiles(lax.bitcast_convert_type(_sll(h, 16) | _sll(nib & 8, 28), F32))


def _lane_level(bad, value):
    return jnp.where(jnp.max(bad, axis=0, keepdims=True) > 0, value, 0)


def _body(x_hbm, out, xin, xw, xr, yw, yr, fw, x0l, x0s, x0r, yls, ylr,
          xs16, xr16, ys16, yr16,
          in_sems, xr_sems, yr_sems, fw_sems, send_sems, p0_sems, slow_sems, dsem):
    mx = lax.axis_index("x")
    my = lax.axis_index("y")
    xn = (1 - mx, my)
    yn = (mx, 1 - my)
    is_a = jnp.logical_and(mx == 0, my == 0)
    is_b = jnp.logical_and(mx == 0, my == 1)
    is_c = jnp.logical_and(mx == 1, my == 0)
    is_d = jnp.logical_and(mx == 1, my == 1)
    own = pl.ds(pl.multiple_of(my * N, N), N)
    oth = pl.ds(pl.multiple_of((1 - my) * N, N), N)

    def rows(p, n=1):
        return pl.ds(p * CH, n * CH)

    def slot(p, header):
        return pl.ds(p * SLOT, HDR + (header(p)[0] == p))

    def read(ref, q, p, header):
        holder, half = header(p)
        row = ref[pl.ds((q + holder - p) * SLOT + HDR, 1), :]
        return _unpack(ref[pl.ds(q * SLOT, HDR), :], _srl(row, 16 * half) & 0xFFFF)

    def remote(src, dst, send_sem, recv_sem, dev):
        return pltpu.make_async_remote_copy(src, dst, send_sem, recv_sem,
                                            device_id=dev, device_id_type=MESH)

    def x_copy(p):
        return remote(xw.at[slot(p, _x_header)], xr.at[slot(p, _x_header)], send_sems.at[0],
                      xr_sems.at[p], xn)

    def y_copy(p):
        if p == LAST:
            return remote(yls, ylr, send_sems.at[3], yr_sems.at[p], yn)
        src = yw if p < KS else xw
        return remote(src.at[slot(p, _y_header)], yr.at[slot(p, _y_header)], send_sems.at[1],
                      yr_sems.at[p], yn)

    def fw_copy(p):
        dst = pl.ds((p - KS) * SLOT, HDR + (_x_header(p)[0] == p))
        return remote(yr.at[slot(p, _x_header)], fw.at[dst], send_sems.at[2],
                      fw_sems.at[p - KS], xn)

    p0a = remote(x_hbm.at[rows(0), pl.ds(0, HALF)], x0l, p0_sems.at[0], p0_sems.at[1], xn)
    p0b = remote(x0s, x0r, p0_sems.at[2], p0_sems.at[3], xn)

    def start_x(ps):
        for p in ps:
            if p == 0:
                p0a.start()
                p0b.start()
            else:
                x_copy(p).start()

    def start_raw():
        for p in range(KS, K):
            y_copy(p).start()

    loads = [pltpu.make_async_copy(x_hbm.at[rows(g[0], len(g))], xin.at[rows(g[0], len(g))],
                                   in_sems.at[i]) for i, g in enumerate(_LOADS)]
    bar = pltpu.get_barrier_semaphore()

    @pl.when(is_c)
    def _():
        pl.semaphore_wait(bar, 1)
        p0a.start()

    loads[0].start()

    @pl.when(jnp.logical_not(is_d))
    def _():
        pl.semaphore_signal(bar, inc=1, device_id=xn, device_id_type=MESH)
        pl.semaphore_signal(bar, inc=1, device_id=yn, device_id_type=MESH)

    for ld in loads[1:]:
        ld.start()

    @pl.when(is_d)
    def _():
        pl.semaphore_wait(bar, 2)
        pl.semaphore_signal(dsem, inc=1, device_id=yn, device_id_type=MESH)
        pl.semaphore_signal(dsem, inc=1, device_id=xn, device_id_type=MESH)
        p0a.start()

    loaded = set()

    def need(p):
        if _LOAD_OF[p] not in loaded:
            loaded.add(_LOAD_OF[p])
            loads[_LOAD_OF[p]].wait()

    def encode_x(ps, bad):
        packed = []
        for p in ps:
            need(p)
            planes, hdr, bad = _pack(xin[rows(p), :], bad)
            packed.append((planes, hdr))
        hdr = packed[0][1]
        if len(ps) == 2:
            hdr = hdr | _sll(packed[1][1], 16)
            xw[pl.ds(ps[1] * SLOT, HDR), :] = packed[1][0]
        elif ps[0] == FLAG:
            hdr = hdr | _lane_level(bad, RAW_BAD)
        xw[pl.ds(ps[0] * SLOT, HDR + 1), :] = jnp.concatenate([packed[0][0], hdr], axis=0)
        return bad

    need(0)
    x0s[...] = xin[rows(0), pl.ds(HALF, HALF)].astype(BF16)

    @pl.when(mx == 1)
    def _():
        p0b.start()

    bad_x = jnp.zeros((8, 128), I32)
    batches = [[1], [2, 3], [4, 5], list(range(KS, K))]
    batches += [list(range(p, min(p + 4, EARLY))) for p in range(6, EARLY, 4)]
    for batch in batches:
        for i in range(0, len(batch), 2):
            bad_x = encode_x(batch[i:i + 2], bad_x)
        if batch[0] < KS:
            @pl.when(mx == 1)
            def _():
                start_x(batch)
        else:
            @pl.when(is_d)
            def _():
                start_raw()

            @pl.when(is_b)
            def _():
                pl.semaphore_wait(bar, 1)
                start_raw()

    @pl.when(is_a)
    def _():
        pl.semaphore_wait(bar, 2)
        start_x([0, 1])
        start_raw()
        start_x(range(2, EARLY))

    @pl.when(is_b)
    def _():
        pl.semaphore_wait(dsem, 1)
        start_x(range(EARLY))

    @pl.when(is_c)
    def _():
        pl.semaphore_wait(dsem, 1)
        start_raw()

    def finish_y(ps):
        for p in ps:
            y_copy(p).wait_recv()
        for p in ps:
            store_y(p)

    def store_y(p):
        got = ylr[...].astype(F32) if p == LAST else read(yr, p, p, _y_header)
        out[rows(p), oth] = got

    def finish_fw(p):
        raw = out[rows(p), oth]
        fw_copy(p).wait_recv()
        out[rows(p), oth] = raw + read(fw, p - KS, p, _x_header)

    def level_of(ref):
        hdr = ref[pl.ds(FLAG * SLOT + HDR, 1), :]
        return jnp.max(_srl(hdr, LEVEL_SHIFT).astype(F32))

    late = [[p, p + 1] for p in range(EARLY, FLAG, 2)] + [[LAST], [FLAG]]
    encoded, next_x, next_y = set(range(EARLY)), EARLY, 0
    bad_y = jnp.zeros((8, 128), I32)
    my_level = held = None
    for p in range(K):
        mine = xin[rows(p), :]
        if p == 0:
            p0a.wait_recv()
            p0b.wait_recv()
            got = jnp.concatenate([x0l[...], x0r[...].astype(F32)], axis=1)
        else:
            x_copy(p).wait_recv()
            got = read(xr, p, p, _x_header)
        s = mine + got
        if p == LAST:
            yls[...] = s.astype(BF16)
        elif p < KS:
            planes, hdr, bad_y = _pack(s, bad_y)
            if p == FLAG:
                hdr_row = pl.ds(p * SLOT + HDR, 1)
                raw_level = (xw[hdr_row, :] | xr[hdr_row, :]) & RAW_BAD
                hdr = hdr | jnp.maximum(_lane_level(bad_y, SUM_BAD), raw_level)
            elif p % 2 == 0:
                held, hdr = hdr, None
            else:
                hdr = held | _sll(hdr, 16)
            if hdr is None:
                yw[pl.ds(p * SLOT, HDR), :] = planes
            else:
                yw[pl.ds(p * SLOT, HDR + 1), :] = jnp.concatenate([planes, hdr], axis=0)
        if p < KS:
            y_copy(p).start()
        out[rows(p), own] = s

        if late and (p % 2 == 0 or len(late[0]) == 1):
            ps = late.pop(0)
            bad_x = encode_x(ps, bad_x)
            encoded.update(ps)
            while next_x in encoded:
                x_copy(next_x).start()
                next_x += 1
            if not late:
                start_x(range(KS, K))
        if p == FWD_AT:
            assert not late
            for q in range(KS, K):
                y_copy(q).wait_recv()
                fw_copy(q).start()
            for q in range(KS, K):
                out[rows(q), oth] = read(yr, q, q, _x_header)
        if next_y < FLAG and next_y + 1 <= p - LAG:
            finish_y([next_y, next_y + 1])
            next_y += 2
        if p == FLAG + 1:
            my_level = level_of(yw)

    finish_fw(KS)
    for p in range(next_y, FLAG, 2):
        finish_y([p, p + 1])
    for p in range(KS + 1, K - 1):
        finish_fw(p)
    finish_y([FLAG])
    in_level = level_of(yr)
    p0a.wait_send()
    p0b.wait_send()
    for p in range(1, K):
        x_copy(p).wait_send()
    for p in range(K):
        y_copy(p).wait_send()
    for p in range(KS, K):
        fw_copy(p).wait_send()
    finish_fw(K - 1)
    finish_y([LAST])

    raw_bad = jnp.maximum(my_level, in_level) >= 2
    send_y = jnp.logical_or(raw_bad, my_level > 0)
    recv_y = jnp.logical_or(raw_bad, in_level > 0)

    @pl.when(jnp.logical_or(send_y, recv_y))
    def _():
        slow_x = remote(xs16, xr16, slow_sems.at[0], slow_sems.at[1], xn)
        slow_y = remote(ys16, yr16, slow_sems.at[2], slow_sems.at[3], yn)

        @pl.when(raw_bad)
        def _():
            xs16[...] = xin[...].astype(BF16)
            slow_x.start()
            slow_x.wait()
            out[:, own] = xin[...] + xr16[...].astype(F32)

        @pl.when(send_y)
        def _():
            ys16[...] = out[:, own].astype(BF16)
            slow_y.start()

        @pl.when(recv_y)
        def _():
            slow_y.wait_recv()
            out[:, oth] = yr16[...].astype(F32)

        @pl.when(send_y)
        def _():
            slow_y.wait_send()


def pallas_dist_redx_gaty_m512_n512_kernel(x: jax.Array):
    dma = pltpu.SemaphoreType.DMA

    def wire(n):
        return pltpu.VMEM((n * SLOT, 128), I32)

    def plain(r, c):
        return pltpu.VMEM((r, c), BF16)

    return pl.pallas_call(
        _body,
        out_shape=pltpu.VMEM((M, 2 * N), F32),
        in_specs=[pl.BlockSpec(memory_space=pl.ANY)],
        out_specs=pl.BlockSpec(memory_space=pltpu.VMEM),
        scratch_shapes=[
            pltpu.VMEM((M, N), F32),
            wire(K), wire(K), wire(KS), wire(K), wire(NR),
            pltpu.VMEM((CH, HALF), F32), plain(CH, HALF), plain(CH, HALF),
            plain(CH, N), plain(CH, N),
            plain(M, N), plain(M, N), plain(M, N), plain(M, N),
            dma((len(_LOADS),)), dma((K,)), dma((K,)), dma((NR,)), dma((4,)),
            dma((4,)), dma((4,)), pltpu.SemaphoreType.REGULAR,
        ],
        compiler_params=pltpu.CompilerParams(collective_id=0, disable_semaphore_checks=True),
    )(x)
```
